```python
import numpy as np

kernel_name = "dist_ag_xy_y_m1024_n512"

def setup_inputs():
    return {"x": np.random.randn(2048, 512).astype(np.float32)}

def reference(x: np.ndarray) -> np.ndarray:
    return x
```

```python
import jax
import jax.numpy as jnp
from jax import lax
from jax.experimental import pallas as pl
from jax.experimental.pallas import tpu as pltpu

_MESH = pl.DeviceIdType.MESH

_CHUNKS = (48,) * 9 + (32,)


def pallas_dist_ag_xy_y_m1024_n512_kernel(
x: jax.Array,
):
    m, n = x.shape
    k_fwd = len(_CHUNKS)
    fwd = sum(_CHUNKS)
    extra = m - 2 * fwd
    offs = [sum(_CHUNKS[:k]) for k in range(k_fwd)]

    def body(x_ref, o_ref, xf, ld_sem, ys_sem, yr_sem, xs_sem, xr_sem):
        mx, my = lax.axis_index("x"), lax.axis_index("y")
        ynbr, xnbr = (mx, 1 - my), (1 - mx, my)
        bar = pltpu.get_barrier_semaphore()
        pl.semaphore_signal(bar, 1, device_id=ynbr, device_id_type=_MESH)
        pl.semaphore_signal(bar, 1, device_id=xnbr, device_id_type=_MESH)

        base = mx * (fwd + extra)
        other = (1 - mx) * (fwd + extra)
        me, th = my * m, (1 - my) * m
        pieces = [(base + offs[k], _CHUNKS[k]) for k in range(k_fwd)] + [(fwd, extra)]
        loads = [
            pltpu.make_async_copy(
                x_ref.at[pl.ds(s, c)], xf.at[pl.ds(s, c)], ld_sem.at[k]
            )
            for k, (s, c) in enumerate(pieces)
        ]
        rest = pltpu.make_async_copy(
            x_ref.at[pl.ds(other, fwd)], xf.at[pl.ds(other, fwd)], ld_sem.at[k_fwd + 1]
        )
        ysend = [
            pltpu.make_async_remote_copy(
                o_ref.at[pl.ds(me + s, c)], o_ref.at[pl.ds(me + s, c)],
                ys_sem.at[k], yr_sem.at[k], device_id=ynbr, device_id_type=_MESH,
            )
            for k, (s, c) in enumerate(pieces)
        ]
        xsend = [
            pltpu.make_async_remote_copy(
                o_ref.at[pl.ds(th + s, c)], o_ref.at[pl.ds(th + s, c)],
                xs_sem.at[k], xr_sem.at[k], device_id=xnbr, device_id_type=_MESH,
            )
            for k, (s, c) in enumerate(pieces[:k_fwd])
        ]
        for l in loads:
            l.start()
        rest.start()
        for k, (s, c) in enumerate(pieces):
            loads[k].wait()
            o_ref[pl.ds(me + s, c), :] = xf[pl.ds(s, c), :].astype(jnp.bfloat16)
            if k == 0:
                pl.semaphore_wait(bar, 2)
            ysend[k].start()
        for k in range(k_fwd):
            ysend[k].wait_recv()
            xsend[k].start()
            if k == 0:
                rest.wait()
                o_ref[pl.ds(me + other, fwd), :] = xf[pl.ds(other, fwd), :].astype(
                    jnp.bfloat16
                )
        for c in ysend[k_fwd:] + xsend:
            c.wait_recv()
        for c in ysend + xsend:
            c.wait_send()

    return pl.pallas_call(
        body,
        out_shape=pltpu.VMEM((2 * m, n), jnp.bfloat16),
        in_specs=[pl.BlockSpec(memory_space=pltpu.HBM)],
        out_specs=pl.BlockSpec(memory_space=pltpu.VMEM),
        scratch_shapes=[
            pltpu.VMEM((m, n), jnp.float32),
            pltpu.SemaphoreType.DMA((k_fwd + 2,)),
            pltpu.SemaphoreType.DMA((k_fwd + 1,)),
            pltpu.SemaphoreType.DMA((k_fwd + 1,)),
            pltpu.SemaphoreType.DMA((k_fwd,)),
            pltpu.SemaphoreType.DMA((k_fwd,)),
        ],
        compiler_params=pltpu.CompilerParams(collective_id=0),
    )(x)
```

```python
import jax
import jax.numpy as jnp
from jax import lax
from jax.experimental import pallas as pl
from jax.experimental.pallas import tpu as pltpu

_MESH = pl.DeviceIdType.MESH

_CHUNK = 48
_N_CHUNKS = 9
_TAIL = (32, 16)
_LOAD_AT = (0, 1, 3, _N_CHUNKS)


def pallas_dist_ag_xy_y_m1024_n512_kernel(
x: jax.Array,
):
    m, n = x.shape
    full = _CHUNK * _N_CHUNKS
    mid_lo, mid_hi = full, m - full
    tail = ((mid_lo, _TAIL[0]), (mid_hi - _TAIL[1], _TAIL[1]))
    direct = (mid_lo + _TAIL[0], mid_hi - mid_lo - sum(_TAIL))
    n_loads = len(_LOAD_AT) - 1

    def body(x_ref, o_ref, xf, ld_sem, ys_sem, yr_sem, xs_sem, xr_sem, entered):
        mx, my = lax.axis_index("x"), lax.axis_index("y")
        y_nbr, x_nbr = (mx, 1 - my), (1 - mx, my)
        mine, theirs = my * m, (1 - my) * m
        sent, kept = mx * mid_hi, (1 - mx) * mid_hi

        def on(px, py):
            return pl.when(jnp.logical_and(mx == px, my == py))

        def signal(sem, device):
            pl.semaphore_signal(sem, 1, device_id=device, device_id_type=_MESH)

        def load(start, rows, i):
            return pltpu.make_async_copy(
                x_ref.at[pl.ds(start, rows)], xf.at[pl.ds(start, rows)], ld_sem.at[i]
            )

        def round_rows(start, rows):
            o_ref[pl.ds(mine + start, rows), :] = xf[pl.ds(start, rows), :].astype(
                jnp.bfloat16
            )

        def y_copy(start, rows, i):
            block = o_ref.at[pl.ds(mine + start, rows)]
            return pltpu.make_async_remote_copy(
                block, block, ys_sem.at[i], yr_sem.at[i],
                device_id=y_nbr, device_id_type=_MESH,
            )

        def y_arrival(start, rows, i):
            block = o_ref.at[pl.ds(theirs + start, rows)]
            return pltpu.make_async_remote_copy(
                block, block, ys_sem.at[i], yr_sem.at[i],
                device_id=y_nbr, device_id_type=_MESH,
            )

        def x_copy(start, rows, i):
            block = o_ref.at[pl.ds(theirs + start, rows)]
            return pltpu.make_async_remote_copy(
                block, block, xs_sem.at[i], xr_sem.at[i],
                device_id=x_nbr, device_id_type=_MESH,
            )

        loads = [
            load(sent + _CHUNK * lo, _CHUNK * (hi - lo), g)
            for g, (lo, hi) in enumerate(zip(_LOAD_AT, _LOAD_AT[1:]))
        ]
        mid_load = load(mid_lo, mid_hi - mid_lo, n_loads)
        kept_load = load(kept, full, n_loads + 1)
        loads[0].start()

        barrier = pltpu.get_barrier_semaphore()
        pl.when(jnp.logical_or(mx == 1, my == 0))(lambda: signal(barrier, y_nbr))
        on(1, 0)(lambda: signal(barrier, x_nbr))
        loads[1].start()
        pl.semaphore_wait(barrier, 1)
        on(0, 1)(lambda: signal(entered, y_nbr))

        @on(0, 0)
        def _():
            pl.semaphore_wait(entered, 1)
            signal(entered, x_nbr)

        for g, (lo, hi) in enumerate(zip(_LOAD_AT, _LOAD_AT[1:])):
            loads[g].wait()
            round_rows(sent + _CHUNK * lo, _CHUNK * (hi - lo))
            for k in range(lo, hi):
                y_copy(sent + _CHUNK * k, _CHUNK, k).start()
            if g == 0:
                for later in loads[2:]:
                    later.start()
                mid_load.start()
            if g == 1:

                @on(1, 0)
                def _():
                    pl.semaphore_wait(entered, 1)
                    signal(entered, y_nbr)
                    signal(entered, (1 - mx, 1 - my))

        mid_load.wait()
        kept_load.start()
        round_rows(mid_lo, mid_hi - mid_lo)
        for px in range(2):
            pl.when(mx == px)(lambda px=px: y_copy(*tail[px], _N_CHUNKS).start())
        y_copy(*direct, _N_CHUNKS + 1).start()

        pl.when(my == 1)(lambda: pl.semaphore_wait(entered, 1))
        for k in range(_N_CHUNKS):
            y_arrival(sent + _CHUNK * k, _CHUNK, k).wait_recv()
            x_copy(sent + _CHUNK * k, _CHUNK, k).start()
            if k == 1:
                kept_load.wait()
                round_rows(kept, full)
        for px in range(2):

            @pl.when(mx == px)
            def _():
                y_arrival(*tail[px], _N_CHUNKS).wait_recv()
                x_copy(*tail[px], _N_CHUNKS).start()

        for k in range(_N_CHUNKS):
            y_copy(sent + _CHUNK * k, _CHUNK, k).wait_send()
            x_copy(sent + _CHUNK * k, _CHUNK, k).wait_send()
            x_copy(kept + _CHUNK * k, _CHUNK, k).wait_recv()
        for px in range(2):

            @pl.when(mx == px)
            def _():
                y_copy(*tail[px], _N_CHUNKS).wait_send()
                x_copy(*tail[px], _N_CHUNKS).wait_send()
                x_copy(*tail[1 - px], _N_CHUNKS).wait_recv()

        y_arrival(*direct, _N_CHUNKS + 1).wait_recv()
        y_copy(*direct, _N_CHUNKS + 1).wait_send()

    return pl.pallas_call(
        body,
        out_shape=pltpu.VMEM((2 * m, n), jnp.bfloat16),
        in_specs=[pl.BlockSpec(memory_space=pltpu.HBM)],
        out_specs=pl.BlockSpec(memory_space=pltpu.VMEM),
        scratch_shapes=[
            pltpu.VMEM((m, n), jnp.float32),
            pltpu.SemaphoreType.DMA((n_loads + 2,)),
            pltpu.SemaphoreType.DMA((_N_CHUNKS + 2,)),
            pltpu.SemaphoreType.DMA((_N_CHUNKS + 2,)),
            pltpu.SemaphoreType.DMA((_N_CHUNKS + 1,)),
            pltpu.SemaphoreType.DMA((_N_CHUNKS + 1,)),
            pltpu.SemaphoreType.REGULAR,
        ],
        compiler_params=pltpu.CompilerParams(collective_id=0),
    )(x)
```
